```python
import numpy as np

kernel_name = "dist_mean_ax0_shard0_i_m1024_n512"

def setup_inputs():
    return {"x": np.random.randn(4096, 512).astype(np.float32)}

def reference(x: np.ndarray) -> np.ndarray:
    return np.mean(x, axis=0, keepdims=True)
```

```python
import jax
import jax.numpy as jnp
from jax import lax
from jax.experimental import pallas as pl
from jax.experimental.pallas import tpu as pltpu

N_DEV = 4
N_CHUNKS = 8


def pallas_dist_mean_ax0_shard0_i_m1024_n512_kernel(
x: jax.Array,
):
    m_per, n = x.shape
    rows = m_per // N_CHUNKS
    inv_total = 1.0 / float(m_per * N_DEV)

    def kernel_body(x_hbm, out_ref, xbuf, part_ref, recv_ref, load_sems, send_sems, recv_sems):
        me = lax.axis_index("i")

        loads = []
        for c in range(N_CHUNKS):
            cp = pltpu.make_async_copy(
                x_hbm.at[pl.ds(c * rows, rows), :],
                xbuf.at[pl.ds(c * rows, rows), :],
                load_sems.at[c],
            )
            cp.start()
            loads.append(cp)

        barrier_sem = pltpu.get_barrier_semaphore()
        for d in range(1, N_DEV):
            pl.semaphore_signal(
                barrier_sem, inc=1,
                device_id=((me + d) % N_DEV,),
                device_id_type=pl.DeviceIdType.MESH,
            )

        acc = jnp.zeros((8, n), jnp.float32)
        for c in range(N_CHUNKS):
            loads[c].wait()
            blk = xbuf[pl.ds(c * rows, rows), :]
            acc = acc + jnp.sum(blk.reshape(rows // 8, 8, n), axis=0)
        part = jnp.sum(acc, axis=0, keepdims=True)
        part_ref[...] = part

        pl.semaphore_wait(barrier_sem, N_DEV - 1)

        rdmas = []
        for d in range(1, N_DEV):
            rdma = pltpu.make_async_remote_copy(
                src_ref=part_ref,
                dst_ref=recv_ref.at[d - 1],
                send_sem=send_sems.at[d - 1],
                recv_sem=recv_sems.at[d - 1],
                device_id=((me + d) % N_DEV,),
                device_id_type=pl.DeviceIdType.MESH,
            )
            rdma.start()
            rdmas.append(rdma)

        total = part
        for d in range(1, N_DEV):
            rdmas[d - 1].wait_recv()
            total = total + recv_ref[d - 1]
        out_ref[...] = total * inv_total

        for d in range(1, N_DEV):
            rdmas[d - 1].wait_send()

    return pl.pallas_call(
        kernel_body,
        out_shape=jax.ShapeDtypeStruct((1, n), jnp.float32),
        in_specs=[pl.BlockSpec(memory_space=pl.ANY)],
        out_specs=pl.BlockSpec(memory_space=pltpu.VMEM),
        scratch_shapes=[
            pltpu.VMEM((m_per, n), jnp.float32),
            pltpu.VMEM((1, n), jnp.float32),
            pltpu.VMEM((N_DEV - 1, 1, n), jnp.float32),
            pltpu.SemaphoreType.DMA((N_CHUNKS,)),
            pltpu.SemaphoreType.DMA((N_DEV - 1,)),
            pltpu.SemaphoreType.DMA((N_DEV - 1,)),
        ],
        compiler_params=pltpu.CompilerParams(collective_id=0),
    )(x)
```

```python
import jax
import jax.numpy as jnp
from jax import lax
from jax.experimental import pallas as pl
from jax.experimental.pallas import tpu as pltpu

N_DEV = 4
MESH = pl.DeviceIdType.MESH

HEAD = (512, 176, 64)
K_OFF = 40
TAIL = 192
N_C = 384
LATE = 2


def _tree(parts):
    while len(parts) > 1:
        nxt = [parts[i] + parts[i + 1] for i in range(0, len(parts) - 1, 2)]
        if len(parts) % 2:
            nxt.append(parts[-1])
        parts = nxt
    return parts[0]


def _tree_rows(ref, acc):
    return _tree(
        [acc] + [ref[pl.ds(8 * i, 8), :] for i in range(ref.shape[0] // 8)]
    )


def _chain_rows(ref, r0, nr):
    blk = ref[pl.ds(r0, nr), :]
    return jnp.sum(blk.reshape(nr // 8, 8, ref.shape[1]), axis=0)


def pallas_dist_mean_ax0_shard0_i_m1024_n512_kernel(
x: jax.Array,
):
    m_per, n = x.shape
    n_d = n - N_C
    k = K_OFF
    n_h = len(HEAD)
    h_off = [sum(HEAD[:i]) for i in range(n_h)]
    o0 = sum(HEAD)
    t0 = o0 + 2 * k
    assert t0 + TAIL == m_per
    inv_total = 1.0 / float(m_per * N_DEV)

    def kernel_body(
        x_hbm, out_ref,
        xbuf, cbuf, dbuf, obuf, pc_ref, pd_ref, recv_c, recv_d,
        load_sems, send_c_sems, recv_c_sems, send_d_sems, recv_d_sems,
        osend_sems, orecv_sem,
    ):
        head_cp = [
            pltpu.make_async_copy(
                x_hbm.at[pl.ds(h_off[i], HEAD[i]), :],
                xbuf.at[pl.ds(h_off[i], HEAD[i]), :],
                load_sems.at[i],
            )
            for i in range(n_h)
        ]
        shared_cp = pltpu.make_async_copy(
            x_hbm.at[pl.ds(o0, 2 * k), :],
            xbuf.at[pl.ds(o0, 2 * k), :],
            load_sems.at[n_h],
        )
        tail_c_cp = pltpu.make_async_copy(
            x_hbm.at[pl.ds(t0, TAIL), pl.ds(0, N_C)], cbuf, load_sems.at[n_h + 1]
        )
        tail_d_cp = pltpu.make_async_copy(
            x_hbm.at[pl.ds(t0, TAIL), pl.ds(N_C, n_d)], dbuf, load_sems.at[n_h + 2]
        )

        head_cp[0].start()
        me = lax.axis_index("i")
        is_late = me == LATE
        not_late = me != LATE
        next_to_late = jnp.bitwise_and(me - LATE, 1) == 1

        def peer(d):
            return jnp.bitwise_and(me + d, N_DEV - 1)

        @pl.when(not_late)
        def _():
            shared_cp.start()

        for cp in head_cp[1:]:
            cp.start()
        tail_c_cp.start()
        tail_d_cp.start()

        barrier_sem = pltpu.get_barrier_semaphore()
        for d in (1, 3, 2):
            pl.semaphore_signal(
                barrier_sem, inc=1, device_id=(peer(d),), device_id_type=MESH
            )

        def ship(j):
            return pltpu.make_async_remote_copy(
                src_ref=x_hbm.at[pl.ds(o0 + j * k, k), :],
                dst_ref=obuf,
                send_sem=osend_sems.at[j],
                recv_sem=orecv_sem,
                device_id=((LATE + (1, 3)[j]) % N_DEV,),
                device_id_type=MESH,
            )

        @pl.when(is_late)
        def _():
            pl.semaphore_wait(barrier_sem, N_DEV - 1)
            ship(0).start()
            ship(1).start()

        zeros = lambda: jnp.zeros((8, n), jnp.float32)

        def own_shared():
            shared_cp.wait()
            return _chain_rows(xbuf, o0, 2 * k)

        def shipped():
            ship(0).wait_recv()
            return _chain_rows(obuf, 0, k)

        head_cp[0].wait()
        acc = _chain_rows(xbuf, h_off[0], HEAD[0])
        acc = acc + lax.cond(not_late, own_shared, zeros)
        for i in range(1, n_h):
            head_cp[i].wait()
            acc = acc + _chain_rows(xbuf, h_off[i], HEAD[i])

        @pl.when(not_late)
        def _():
            pl.semaphore_wait(barrier_sem, N_DEV - 1)

        acc = acc + lax.cond(next_to_late, shipped, zeros)

        def rdma_c(d):
            return pltpu.make_async_remote_copy(
                src_ref=pc_ref,
                dst_ref=recv_c.at[d - 1],
                send_sem=send_c_sems.at[d - 1],
                recv_sem=recv_c_sems.at[d - 1],
                device_id=(peer(d),),
                device_id_type=MESH,
            )

        def rdma_d(d):
            return pltpu.make_async_remote_copy(
                src_ref=pd_ref,
                dst_ref=recv_d.at[d - 1],
                send_sem=send_d_sems.at[d - 1],
                recv_sem=recv_d_sems.at[d - 1],
                device_id=(peer(d),),
                device_id_type=MESH,
            )

        tail_c_cp.wait()
        acc_c = _tree_rows(cbuf, acc[:, :N_C])
        pc_ref[...] = jnp.sum(acc_c, axis=0, keepdims=True) * inv_total
        rdma_c(2).start()

        tail_d_cp.wait()
        acc_d = _tree_rows(dbuf, acc[:, N_C:])
        pd_ref[...] = jnp.sum(acc_d, axis=0, keepdims=True) * inv_total
        rdma_d(2).start()
        for d in (1, 3):
            rdma_c(d).start()
            rdma_d(d).start()

        for d in (2, 1, 3):
            rdma_c(d).wait_send()
            rdma_d(d).wait_send()

        @pl.when(is_late)
        def _():
            ship(0).wait_send()
            ship(1).wait_send()

        tot_c = pc_ref[...]
        tot_d = pd_ref[...]
        for d in (1, 3):
            rdma_c(d).wait_recv()
            tot_c = tot_c + recv_c[d - 1]
            rdma_d(d).wait_recv()
            tot_d = tot_d + recv_d[d - 1]
        rdma_c(2).wait_recv()
        out_ref[:, pl.ds(0, N_C)] = tot_c + recv_c[1]
        rdma_d(2).wait_recv()
        out_ref[:, pl.ds(N_C, n_d)] = tot_d + recv_d[1]

    return pl.pallas_call(
        kernel_body,
        out_shape=jax.ShapeDtypeStruct((1, n), jnp.float32),
        in_specs=[pl.BlockSpec(memory_space=pl.ANY)],
        out_specs=pl.BlockSpec(memory_space=pltpu.VMEM),
        scratch_shapes=[
            pltpu.VMEM((t0, n), jnp.float32),
            pltpu.VMEM((TAIL, N_C), jnp.float32),
            pltpu.VMEM((TAIL, n_d), jnp.float32),
            pltpu.VMEM((k, n), jnp.float32),
            pltpu.VMEM((1, N_C), jnp.float32),
            pltpu.VMEM((1, n_d), jnp.float32),
            pltpu.VMEM((N_DEV - 1, 1, N_C), jnp.float32),
            pltpu.VMEM((N_DEV - 1, 1, n_d), jnp.float32),
            pltpu.SemaphoreType.DMA((n_h + 3,)),
            pltpu.SemaphoreType.DMA((N_DEV - 1,)),
            pltpu.SemaphoreType.DMA((N_DEV - 1,)),
            pltpu.SemaphoreType.DMA((N_DEV - 1,)),
            pltpu.SemaphoreType.DMA((N_DEV - 1,)),
            pltpu.SemaphoreType.DMA((2,)),
            pltpu.SemaphoreType.DMA,
        ],
        compiler_params=pltpu.CompilerParams(
            collective_id=0,
            disable_semaphore_checks=True,
        ),
    )(x)
```

```python
import jax
import jax.numpy as jnp
from jax import lax
from jax.experimental import pallas as pl
from jax.experimental.pallas import tpu as pltpu

N_DEV = 4
MESH = pl.DeviceIdType.MESH

HEAD = (512, 176, 64)
K_OFF = 40
TAIL = 192
N_C = 384
LATE = 2


def _compiler_params():
    try:
        return pltpu.CompilerParams(collective_id=0, disable_semaphore_checks=True)
    except TypeError:
        return pltpu.CompilerParams(collective_id=0)


def _tree(parts):
    while len(parts) > 1:
        nxt = [parts[i] + parts[i + 1] for i in range(0, len(parts) - 1, 2)]
        if len(parts) % 2:
            nxt.append(parts[-1])
        parts = nxt
    return parts[0]


def _tree_rows(ref, acc):
    return _tree(
        [acc] + [ref[pl.ds(8 * i, 8), :] for i in range(ref.shape[0] // 8)]
    )


def _chain_rows(ref, r0, nr):
    blk = ref[pl.ds(r0, nr), :]
    return jnp.sum(blk.reshape(nr // 8, 8, ref.shape[1]), axis=0)


def pallas_dist_mean_ax0_shard0_i_m1024_n512_kernel(
x: jax.Array,
):
    m_per, n = x.shape
    n_d = n - N_C
    k = K_OFF
    n_h = len(HEAD)
    h_off = [sum(HEAD[:i]) for i in range(n_h)]
    o0 = sum(HEAD)
    t0 = o0 + 2 * k
    assert t0 + TAIL == m_per
    inv_total = 1.0 / float(m_per * N_DEV)

    def kernel_body(
        x_hbm, out_ref,
        xbuf, cbuf, dbuf, obuf, pc_ref, pd_ref, recv_c, recv_d,
        load_sems, send_c_sems, recv_c_sems, send_d_sems, recv_d_sems,
        osend_sems, orecv_sem,
    ):
        head_cp = [
            pltpu.make_async_copy(
                x_hbm.at[pl.ds(h_off[i], HEAD[i]), :],
                xbuf.at[pl.ds(h_off[i], HEAD[i]), :],
                load_sems.at[i],
            )
            for i in range(n_h)
        ]
        shared_cp = pltpu.make_async_copy(
            x_hbm.at[pl.ds(o0, 2 * k), :],
            xbuf.at[pl.ds(o0, 2 * k), :],
            load_sems.at[n_h],
        )
        tail_c_cp = pltpu.make_async_copy(
            x_hbm.at[pl.ds(t0, TAIL), pl.ds(0, N_C)], cbuf, load_sems.at[n_h + 1]
        )
        tail_d_cp = pltpu.make_async_copy(
            x_hbm.at[pl.ds(t0, TAIL), pl.ds(N_C, n_d)], dbuf, load_sems.at[n_h + 2]
        )

        head_cp[0].start()
        me = lax.axis_index("i")
        is_late = me == LATE
        not_late = me != LATE
        next_to_late = jnp.bitwise_and(me - LATE, 1) == 1

        def peer(d):
            return jnp.bitwise_and(me + d, N_DEV - 1)

        @pl.when(not_late)
        def _():
            shared_cp.start()

        for cp in head_cp[1:]:
            cp.start()
        tail_c_cp.start()
        tail_d_cp.start()

        barrier_sem = pltpu.get_barrier_semaphore()
        for d in (1, 3, 2):
            pl.semaphore_signal(
                barrier_sem, inc=1, device_id=(peer(d),), device_id_type=MESH
            )

        def ship(j):
            return pltpu.make_async_remote_copy(
                src_ref=x_hbm.at[pl.ds(o0 + j * k, k), :],
                dst_ref=obuf,
                send_sem=osend_sems.at[j],
                recv_sem=orecv_sem,
                device_id=((LATE + (1, 3)[j]) % N_DEV,),
                device_id_type=MESH,
            )

        @pl.when(is_late)
        def _():
            pl.semaphore_wait(barrier_sem, N_DEV - 1)
            ship(0).start()
            ship(1).start()

        zeros = lambda: jnp.zeros((8, n), jnp.float32)

        def own_shared():
            shared_cp.wait()
            return _chain_rows(xbuf, o0, 2 * k)

        def shipped():
            ship(0).wait_recv()
            return _chain_rows(obuf, 0, k)

        head_cp[0].wait()
        acc = _chain_rows(xbuf, h_off[0], HEAD[0])
        acc = acc + lax.cond(not_late, own_shared, zeros)
        for i in range(1, n_h):
            head_cp[i].wait()
            acc = acc + _chain_rows(xbuf, h_off[i], HEAD[i])

        @pl.when(not_late)
        def _():
            pl.semaphore_wait(barrier_sem, N_DEV - 1)

        acc = acc + lax.cond(next_to_late, shipped, zeros)

        def rdma_c(d):
            return pltpu.make_async_remote_copy(
                src_ref=pc_ref,
                dst_ref=recv_c.at[d - 1],
                send_sem=send_c_sems.at[d - 1],
                recv_sem=recv_c_sems.at[d - 1],
                device_id=(peer(d),),
                device_id_type=MESH,
            )

        def rdma_d(d):
            return pltpu.make_async_remote_copy(
                src_ref=pd_ref,
                dst_ref=recv_d.at[d - 1],
                send_sem=send_d_sems.at[d - 1],
                recv_sem=recv_d_sems.at[d - 1],
                device_id=(peer(d),),
                device_id_type=MESH,
            )

        tail_c_cp.wait()
        acc_c = _tree_rows(cbuf, acc[:, :N_C])
        pc_ref[...] = jnp.sum(acc_c, axis=0, keepdims=True) * inv_total
        rdma_c(2).start()

        tail_d_cp.wait()
        acc_d = _tree_rows(dbuf, acc[:, N_C:])
        pd_ref[...] = jnp.sum(acc_d, axis=0, keepdims=True) * inv_total
        rdma_d(2).start()
        for d in (1, 3):
            rdma_c(d).start()
            rdma_d(d).start()

        for d in (2, 1, 3):
            rdma_c(d).wait_send()
            rdma_d(d).wait_send()

        @pl.when(is_late)
        def _():
            ship(0).wait_send()
            ship(1).wait_send()

        tot_c = pc_ref[...]
        tot_d = pd_ref[...]
        for d in (1, 3):
            rdma_c(d).wait_recv()
            tot_c = tot_c + recv_c[d - 1]
            rdma_d(d).wait_recv()
            tot_d = tot_d + recv_d[d - 1]
        rdma_c(2).wait_recv()
        out_ref[:, pl.ds(0, N_C)] = tot_c + recv_c[1]
        rdma_d(2).wait_recv()
        out_ref[:, pl.ds(N_C, n_d)] = tot_d + recv_d[1]

    return pl.pallas_call(
        kernel_body,
        out_shape=jax.ShapeDtypeStruct((1, n), jnp.float32),
        in_specs=[pl.BlockSpec(memory_space=pl.ANY)],
        out_specs=pl.BlockSpec(memory_space=pltpu.VMEM),
        scratch_shapes=[
            pltpu.VMEM((t0, n), jnp.float32),
            pltpu.VMEM((TAIL, N_C), jnp.float32),
            pltpu.VMEM((TAIL, n_d), jnp.float32),
            pltpu.VMEM((k, n), jnp.float32),
            pltpu.VMEM((1, N_C), jnp.float32),
            pltpu.VMEM((1, n_d), jnp.float32),
            pltpu.VMEM((N_DEV - 1, 1, N_C), jnp.float32),
            pltpu.VMEM((N_DEV - 1, 1, n_d), jnp.float32),
            pltpu.SemaphoreType.DMA((n_h + 3,)),
            pltpu.SemaphoreType.DMA((N_DEV - 1,)),
            pltpu.SemaphoreType.DMA((N_DEV - 1,)),
            pltpu.SemaphoreType.DMA((N_DEV - 1,)),
            pltpu.SemaphoreType.DMA((N_DEV - 1,)),
            pltpu.SemaphoreType.DMA((2,)),
            pltpu.SemaphoreType.DMA,
        ],
        compiler_params=_compiler_params(),
    )(x)
```
